```python
import numpy as np

kernel_name = "dist_mean_ax0_shard0_i_m1024_n512"

def setup_inputs():
    return {"x": np.random.randn(4096, 512).astype(np.float32)}

def reference(x: np.ndarray) -> np.ndarray:
    return np.mean(x, axis=0, keepdims=True)
```

```python
import jax
import jax.numpy as jnp
from jax import lax
from jax.experimental import pallas as pl
from jax.experimental.pallas import tpu as pltpu

N_DEV = 4
N_CHUNKS = 4


def pallas_dist_mean_ax0_shard0_i_m1024_n512_kernel(
x: jax.Array,
):
    m, n = x.shape
    rows = m // N_CHUNKS
    inv_count = 1.0 / (m * N_DEV)

    def kernel_body(x_hbm, out_ref, x_vmem, comm, load_sems, send_sems, recv_sems):
        me = lax.axis_index("i")

        loads = [
            pltpu.make_async_copy(
                x_hbm.at[pl.ds(c * rows, rows)],
                x_vmem.at[pl.ds(c * rows, rows)],
                load_sems.at[c],
            )
            for c in range(N_CHUNKS)
        ]
        for load in loads:
            load.start()

        barrier = pltpu.get_barrier_semaphore()
        for d in range(1, N_DEV):
            pl.semaphore_signal(
                barrier, inc=1,
                device_id=((me + d) % N_DEV,),
                device_id_type=pl.DeviceIdType.MESH,
            )

        acc = None
        for c in range(N_CHUNKS):
            loads[c].wait()
            blk = x_vmem[pl.ds(c * rows, rows), :].reshape(rows // 8, 8, n)
            part = jnp.sum(blk, axis=0)
            acc = part if acc is None else acc + part
        comm[0] = jnp.sum(acc, axis=0, keepdims=True)

        pl.semaphore_wait(barrier, N_DEV - 1)

        sends = [
            pltpu.make_async_remote_copy(
                src_ref=comm.at[0],
                dst_ref=comm.at[d],
                send_sem=send_sems.at[d - 1],
                recv_sem=recv_sems.at[d - 1],
                device_id=((me + d) % N_DEV,),
                device_id_type=pl.DeviceIdType.MESH,
            )
            for d in (2, 1, 3)
        ]
        for s in sends:
            s.start()
        for s in sends:
            s.wait_recv()
        out_ref[...] = ((comm[0] + comm[2]) + (comm[1] + comm[3])) * inv_count
        for s in sends:
            s.wait_send()

    return pl.pallas_call(
        kernel_body,
        out_shape=jax.ShapeDtypeStruct((1, n), jnp.float32),
        in_specs=[pl.BlockSpec(memory_space=pl.ANY)],
        out_specs=pl.BlockSpec(memory_space=pltpu.VMEM),
        scratch_shapes=[
            pltpu.VMEM((m, n), jnp.float32),
            pltpu.VMEM((N_DEV, 1, n), jnp.float32),
            pltpu.SemaphoreType.DMA((N_CHUNKS,)),
            pltpu.SemaphoreType.DMA((N_DEV - 1,)),
            pltpu.SemaphoreType.DMA((N_DEV - 1,)),
        ],
        compiler_params=pltpu.CompilerParams(collective_id=0),
    )(x)
```

```python
import jax
import jax.numpy as jnp
from jax import lax
from jax.experimental import pallas as pl
from jax.experimental.pallas import tpu as pltpu

N_DEV = 4
SUBLANES = 8
LANES = 128

DIAGONAL = 2
NEIGHBOURS = (1, 3)

LAST_CHIP = 2
HANDOFF_ROWS = 40

TAIL_CHUNKS = (64, 8)

WIRE_DTYPE = jnp.bfloat16


def _sum_row_groups(ref, start, rows):
    sums = [None, None]
    for g in range(rows // SUBLANES):
        group = ref[pl.ds(start + g * SUBLANES, SUBLANES), :]
        sums[g % 2] = group if sums[g % 2] is None else sums[g % 2] + group
    return sums[0] if sums[1] is None else sums[0] + sums[1]


def _column_sums(acc):
    total = jnp.sum(acc, axis=0, keepdims=True)
    blocks = [total[:, j:j + LANES] for j in range(0, acc.shape[1], LANES)]
    return jnp.concatenate(blocks, axis=0)


def pallas_dist_mean_ax0_shard0_i_m1024_n512_kernel(
x: jax.Array,
):
    m, n = x.shape
    inv_count = 1.0 / (N_DEV * m)
    own_rows = m - len(NEIGHBOURS) * HANDOFF_ROWS
    chunk_rows = (own_rows - sum(TAIL_CHUNKS),) + TAIL_CHUNKS
    chunk_starts = [sum(chunk_rows[:c]) for c in range(len(chunk_rows))]
    folded = (n // LANES, LANES)

    def kernel_body(
        x_hbm, out_ref,
        x_vmem, handed, extra, mine, from_1, from_2, from_3,
        load_sems, rest_sem, send_sems, recv_sems, hand_send_sems, hand_recv_sem,
    ):
        loads = [
            pltpu.make_async_copy(
                x_hbm.at[pl.ds(start, rows)],
                x_vmem.at[pl.ds(start, rows)],
                load_sems.at[c],
            )
            for c, (start, rows) in enumerate(zip(chunk_starts, chunk_rows))
        ]
        for load in loads:
            load.start()

        me = lax.axis_index("i")
        role = me ^ LAST_CHIP
        is_last = role == 0
        not_last = role != 0
        next_to_last = (role & 1) == 1

        def peer(d):
            return dict(device_id=(me ^ d,), device_id_type=pl.DeviceIdType.MESH)

        load_rest = pltpu.make_async_copy(
            x_hbm.at[pl.ds(own_rows, m - own_rows)],
            x_vmem.at[pl.ds(own_rows, m - own_rows)],
            rest_sem,
        )

        @pl.when(not_last)
        def _():
            load_rest.start()

        barrier = pltpu.get_barrier_semaphore()
        for d in (DIAGONAL,) + NEIGHBOURS:
            pl.semaphore_signal(barrier, inc=1, **peer(d))
        pl.semaphore_wait(barrier, N_DEV - 1)

        handoffs = [
            pltpu.make_async_remote_copy(
                src_ref=x_hbm.at[pl.ds(own_rows + j * HANDOFF_ROWS, HANDOFF_ROWS)],
                dst_ref=handed,
                send_sem=hand_send_sems.at[j],
                recv_sem=hand_recv_sem,
                **peer(d),
            )
            for j, d in enumerate(NEIGHBOURS)
        ]

        @pl.when(is_last)
        def _():
            for handoff in handoffs:
                handoff.start()

        extra[...] = jnp.zeros(extra.shape, extra.dtype)

        acc = None
        for c, (start, rows) in enumerate(zip(chunk_starts, chunk_rows)):
            if c == len(loads) - 1:
                @pl.when(not_last)
                def _():
                    load_rest.wait()
                    extra[...] = _sum_row_groups(x_vmem, own_rows, m - own_rows)

                @pl.when(next_to_last)
                def _():
                    handoffs[0].wait_recv()
                    extra[...] += _sum_row_groups(handed, 0, HANDOFF_ROWS)

                acc = acc + extra[...]
            loads[c].wait()
            part = _sum_row_groups(x_vmem, start, rows)
            acc = part if acc is None else acc + part

        mine[...] = (_column_sums(acc) * inv_count).astype(WIRE_DTYPE)

        inbox = {1: from_1, 2: from_2, 3: from_3}
        exchange = {
            d: pltpu.make_async_remote_copy(
                src_ref=mine,
                dst_ref=inbox[d],
                send_sem=send_sems.at[d - 1],
                recv_sem=recv_sems.at[d - 1],
                **peer(d),
            )
            for d in (DIAGONAL,) + NEIGHBOURS
        }
        for d in (DIAGONAL,) + NEIGHBOURS:
            exchange[d].start()

        @pl.when(is_last)
        def _():
            for handoff in handoffs:
                handoff.wait_send()

        for d in NEIGHBOURS:
            exchange[d].wait_recv()
        for d in NEIGHBOURS + (DIAGONAL,):
            exchange[d].wait_send()

        near = mine[...].astype(jnp.float32) + from_1[...].astype(jnp.float32)
        third = from_3[...].astype(jnp.float32)
        exchange[DIAGONAL].wait_recv()
        out_ref[...] = near + (third + from_2[...].astype(jnp.float32))

    out = pl.pallas_call(
        kernel_body,
        out_shape=jax.ShapeDtypeStruct(folded, jnp.float32),
        in_specs=[pl.BlockSpec(memory_space=pltpu.HBM)],
        out_specs=pl.BlockSpec(memory_space=pltpu.VMEM),
        scratch_shapes=[
            pltpu.VMEM((m, n), jnp.float32),
            pltpu.VMEM((HANDOFF_ROWS, n), jnp.float32),
            pltpu.VMEM((SUBLANES, n), jnp.float32),
            pltpu.VMEM(folded, WIRE_DTYPE),
            pltpu.VMEM(folded, WIRE_DTYPE),
            pltpu.VMEM(folded, WIRE_DTYPE),
            pltpu.VMEM(folded, WIRE_DTYPE),
            pltpu.SemaphoreType.DMA((len(chunk_rows),)),
            pltpu.SemaphoreType.DMA,
            pltpu.SemaphoreType.DMA((N_DEV - 1,)),
            pltpu.SemaphoreType.DMA((N_DEV - 1,)),
            pltpu.SemaphoreType.DMA((len(NEIGHBOURS),)),
            pltpu.SemaphoreType.DMA,
        ],
        compiler_params=pltpu.CompilerParams(
            collective_id=0,
            disable_semaphore_checks=True,
        ),
    )(x)
    return out.reshape(1, n)
```
